```python
import numpy as np

kernel_name = "dist_mean_ax0_shard0_i_m2048_n1024"

def setup_inputs():
    return {"x": np.random.randn(8192, 1024).astype(np.float32)}

def reference(x: np.ndarray) -> np.ndarray:
    return np.mean(x, axis=0, keepdims=True)
```

```python
import jax
import jax.numpy as jnp
from jax import lax
from jax.experimental import pallas as pl
from jax.experimental.pallas import tpu as pltpu

N_DEV = 4
CHUNK_ROWS = 256


def pallas_dist_mean_ax0_shard0_i_m2048_n1024_kernel(
x: jax.Array,
):
    m, n = x.shape
    n_chunks = m // CHUNK_ROWS
    scale = 1.0 / (m * N_DEV)

    def kernel_body(x_hbm, out_ref, buf, parts, load_sems, send_sems, recv_sems):
        me = lax.axis_index("i")

        def load(c):
            rows = pl.ds(c * CHUNK_ROWS, CHUNK_ROWS)
            return pltpu.make_async_copy(x_hbm.at[rows], buf.at[rows], load_sems.at[c])

        for c in range(n_chunks):
            load(c).start()

        barrier = pltpu.get_barrier_semaphore()
        for d in range(1, N_DEV):
            pl.semaphore_signal(
                barrier, inc=1, device_id=((me + d) % N_DEV,),
                device_id_type=pl.DeviceIdType.MESH,
            )

        acc = jnp.zeros((8, n), jnp.float32)
        for c in range(n_chunks):
            load(c).wait()
            blk = buf[pl.ds(c * CHUNK_ROWS, CHUNK_ROWS), :]
            acc = acc + jnp.sum(blk.reshape(CHUNK_ROWS // 8, 8, n), axis=0)
        parts[0] = jnp.sum(acc, axis=0, keepdims=True)

        pl.semaphore_wait(barrier, N_DEV - 1)

        def send(d):
            return pltpu.make_async_remote_copy(
                src_ref=parts.at[0], dst_ref=parts.at[d],
                send_sem=send_sems.at[d], recv_sem=recv_sems.at[d],
                device_id=((me + d) % N_DEV,), device_id_type=pl.DeviceIdType.MESH,
            )

        for d in (2, 1, 3):
            send(d).start()
        for d in (1, 3, 2):
            send(d).wait_recv()
        out_ref[...] = ((parts[0] + parts[1]) + (parts[2] + parts[3])) * scale
        for d in (2, 1, 3):
            send(d).wait_send()

    return pl.pallas_call(
        kernel_body,
        out_shape=jax.ShapeDtypeStruct((1, n), jnp.float32),
        in_specs=[pl.BlockSpec(memory_space=pl.ANY)],
        out_specs=pl.BlockSpec(memory_space=pltpu.VMEM),
        scratch_shapes=[
            pltpu.VMEM((m, n), jnp.float32),
            pltpu.VMEM((N_DEV, 1, n), jnp.float32),
            pltpu.SemaphoreType.DMA((n_chunks,)),
            pltpu.SemaphoreType.DMA((N_DEV,)),
            pltpu.SemaphoreType.DMA((N_DEV,)),
        ],
        compiler_params=pltpu.CompilerParams(
            collective_id=0, vmem_limit_bytes=32 * 1024 * 1024
        ),
    )(x)
```

```python
import jax
import jax.numpy as jnp
from jax import lax
from jax.experimental import pallas as pl
from jax.experimental.pallas import tpu as pltpu

N_DEV = 4
SUBLANES, LANES = 8, 128
RIGHT, DIAGONAL, LEFT = 1, 2, 3

SHARED_ROWS = 96
MID_ROWS = 88
TAIL_ROWS = 128
LAST_WIDE_ROWS = 8


def _tree_sum(terms):
    while len(terms) > 1:
        pairs = [a + b for a, b in zip(terms[0::2], terms[1::2])]
        terms = pairs + terms[2 * len(pairs):]
    return terms[0]


def pallas_dist_mean_ax0_shard0_i_m2048_n1024_kernel(
x: jax.Array,
):
    m, n = x.shape
    shared = 2 * SHARED_ROWS
    tail = m - TAIL_ROWS
    mid = tail - MID_ROWS
    last = m - LAST_WIDE_ROWS
    assert m % SUBLANES == 0 and n % LANES == 0 and n > LANES and shared < mid
    wide, strip, every = pl.ds(0, n - LANES), pl.ds(n - LANES, LANES), pl.ds(0, n)
    blocks = (
        (pl.ds(shared, mid - shared), every),
        (pl.ds(mid, MID_ROWS), every),
        (pl.ds(tail, last - tail), wide),
        (pl.ds(last, LAST_WIDE_ROWS), wide),
        (pl.ds(tail, TAIL_ROWS), strip),
    )

    def kernel_body(x_hbm, out_ref, rows, parts, load_sems, send_sems, recv_sems):
        loads = [
            pltpu.make_async_copy(x_hbm.at[b], rows.at[b], load_sems.at[k])
            for k, b in enumerate(blocks)
        ]
        for load in loads:
            load.start()

        me = lax.axis_index("i")
        peer = {d: (me + d) & (N_DEV - 1) for d in (RIGHT, LEFT, DIAGONAL)}

        def push(k, d, src, dst):
            return pltpu.make_async_remote_copy(
                src_ref=src, dst_ref=dst,
                send_sem=send_sems.at[k], recv_sem=recv_sems.at[k],
                device_id=(peer[d],), device_id_type=pl.DeviceIdType.MESH,
            )

        def push_rows(k, d):
            r = pl.ds(k * SHARED_ROWS, SHARED_ROWS)
            return push(k, d, x_hbm.at[r], rows.at[r])

        def push_part(k, d, cols):
            return push(k, d, parts.at[0, :, cols], parts.at[d, :, cols])

        shared_rows = (push_rows(0, RIGHT), push_rows(1, LEFT))
        far_wide = push_part(2, DIAGONAL, wide)
        far_strip = push_part(3, DIAGONAL, strip)
        near = (push_part(4, RIGHT, every), push_part(5, LEFT, every))

        barrier = pltpu.get_barrier_semaphore()
        for p in peer.values():
            pl.semaphore_signal(
                barrier, inc=1, device_id=(p,), device_id_type=pl.DeviceIdType.MESH
            )
        pl.semaphore_wait(barrier, N_DEV - 1)
        for copy in shared_rows:
            copy.start()

        def fold(r, cols):
            v = rows[r, cols]
            return jnp.sum(v.reshape(-1, SUBLANES, v.shape[1]), axis=0)

        def load_and_fold(k):
            loads[k].wait()
            return fold(*blocks[k])

        acc = load_and_fold(0)
        acc += load_and_fold(1)
        for copy in shared_rows:
            copy.wait_recv()
        acc += fold(pl.ds(0, shared), every)

        acc_wide = acc[:, : n - LANES] + load_and_fold(2)
        acc_wide += load_and_fold(3)
        parts[0, :, wide] = jnp.sum(acc_wide, axis=0, keepdims=True)
        far_wide.start()

        loads[4].wait()
        acc_strip = _tree_sum(
            [rows[pl.ds(r, SUBLANES), strip] for r in range(tail, m, SUBLANES)]
            + [acc[:, n - LANES :]]
        )
        parts[0, :, strip] = jnp.sum(acc_strip, axis=0, keepdims=True)
        far_strip.start()
        for copy in near:
            copy.start()

        for copy in (*shared_rows, far_wide, far_strip, *near):
            copy.wait_send()
        for copy in near:
            copy.wait_recv()
        own, neighbours = parts[0], parts[RIGHT] + parts[LEFT]
        far_wide.wait_recv()
        far_strip.wait_recv()
        total = (own + parts[DIAGONAL]) + neighbours
        out_ref[...] = total * (1.0 / (m * N_DEV))

    return pl.pallas_call(
        kernel_body,
        out_shape=jax.ShapeDtypeStruct((1, n), jnp.float32),
        in_specs=[pl.BlockSpec(memory_space=pl.ANY)],
        out_specs=pl.BlockSpec(memory_space=pltpu.VMEM),
        scratch_shapes=[
            pltpu.VMEM((m, n), jnp.float32),
            pltpu.VMEM((N_DEV, 1, n), jnp.float32),
            pltpu.SemaphoreType.DMA((len(blocks),)),
            pltpu.SemaphoreType.DMA((6,)),
            pltpu.SemaphoreType.DMA((6,)),
        ],
        compiler_params=pltpu.CompilerParams(
            collective_id=0,
            disable_semaphore_checks=True,
        ),
    )(x)
```

```python
import jax
import jax.numpy as jnp
from jax import lax
from jax.experimental import pallas as pl
from jax.experimental.pallas import tpu as pltpu

N_DEV = 4
SUBLANES, LANES = 8, 128
RIGHT, DIAGONAL, LEFT = 1, 2, 3

SHARED_ROWS = 96
TAIL_ROWS = 128
LAST_WIDE_ROWS = 8


def _tree_sum(terms):
    while len(terms) > 1:
        pairs = [a + b for a, b in zip(terms[0::2], terms[1::2])]
        terms = pairs + terms[2 * len(pairs):]
    return terms[0]


def pallas_dist_mean_ax0_shard0_i_m2048_n1024_kernel(
x: jax.Array,
):
    m, n = x.shape
    shared = 2 * SHARED_ROWS
    tail = m - TAIL_ROWS
    last = m - LAST_WIDE_ROWS
    assert m % SUBLANES == 0 and n % LANES == 0 and n > LANES and shared < tail
    wide, strip, every = pl.ds(0, n - LANES), pl.ds(n - LANES, LANES), pl.ds(0, n)
    blocks = (
        (pl.ds(shared, tail - shared), every),
        (pl.ds(tail, last - tail), wide),
        (pl.ds(last, LAST_WIDE_ROWS), wide),
        (pl.ds(tail, TAIL_ROWS), strip),
    )

    def kernel_body(x_hbm, out_ref, rows, parts, load_sems, send_sems, recv_sems):
        loads = [
            pltpu.make_async_copy(x_hbm.at[b], rows.at[b], load_sems.at[k])
            for k, b in enumerate(blocks)
        ]
        for load in loads:
            load.start()

        me = lax.axis_index("i")
        peer = {d: (me + d) & (N_DEV - 1) for d in (RIGHT, LEFT, DIAGONAL)}

        def push(k, d, src, dst):
            return pltpu.make_async_remote_copy(
                src_ref=src, dst_ref=dst,
                send_sem=send_sems.at[k], recv_sem=recv_sems.at[k],
                device_id=(peer[d],), device_id_type=pl.DeviceIdType.MESH,
            )

        def push_rows(k, d):
            r = pl.ds(k * SHARED_ROWS, SHARED_ROWS)
            return push(k, d, x_hbm.at[r], rows.at[r])

        def push_part(k, d, cols):
            return push(k, d, parts.at[0, :, cols], parts.at[d, :, cols])

        shared_rows = (push_rows(0, RIGHT), push_rows(1, LEFT))
        far_wide = push_part(2, DIAGONAL, wide)
        far_strip = push_part(3, DIAGONAL, strip)
        near = (push_part(4, RIGHT, every), push_part(5, LEFT, every))

        barrier = pltpu.get_barrier_semaphore()
        for p in peer.values():
            pl.semaphore_signal(
                barrier, inc=1, device_id=(p,), device_id_type=pl.DeviceIdType.MESH
            )
        pl.semaphore_wait(barrier, N_DEV - 1)
        for copy in shared_rows:
            copy.start()

        def fold(r, cols):
            v = rows[r, cols]
            return jnp.sum(v.reshape(-1, SUBLANES, v.shape[1]), axis=0)

        def load_and_fold(k):
            loads[k].wait()
            return fold(*blocks[k])

        acc = load_and_fold(0)
        for copy in shared_rows:
            copy.wait_recv()
        acc += fold(pl.ds(0, shared), every)

        acc_wide = acc[:, : n - LANES] + load_and_fold(1)
        acc_wide += load_and_fold(2)
        parts[0, :, wide] = jnp.sum(acc_wide, axis=0, keepdims=True)
        far_wide.start()

        loads[3].wait()
        acc_strip = _tree_sum(
            [rows[pl.ds(r, SUBLANES), strip] for r in range(tail, m, SUBLANES)]
            + [acc[:, n - LANES :]]
        )
        parts[0, :, strip] = jnp.sum(acc_strip, axis=0, keepdims=True)
        far_strip.start()
        for copy in near:
            copy.start()

        for copy in (*shared_rows, far_wide, far_strip, *near):
            copy.wait_send()
        for copy in near:
            copy.wait_recv()
        own, neighbours = parts[0], parts[RIGHT] + parts[LEFT]
        far_wide.wait_recv()
        far_strip.wait_recv()
        total = (own + parts[DIAGONAL]) + neighbours
        out_ref[...] = total * (1.0 / (m * N_DEV))

    return pl.pallas_call(
        kernel_body,
        out_shape=jax.ShapeDtypeStruct((1, n), jnp.float32),
        in_specs=[pl.BlockSpec(memory_space=pl.ANY)],
        out_specs=pl.BlockSpec(memory_space=pltpu.VMEM),
        scratch_shapes=[
            pltpu.VMEM((m, n), jnp.float32),
            pltpu.VMEM((N_DEV, 1, n), jnp.float32),
            pltpu.SemaphoreType.DMA((len(blocks),)),
            pltpu.SemaphoreType.DMA((6,)),
            pltpu.SemaphoreType.DMA((6,)),
        ],
        compiler_params=pltpu.CompilerParams(
            collective_id=0,
            disable_semaphore_checks=True,
        ),
    )(x)
```
